```python
import numpy as np

kernel_name = "dist_mean_ax0_xy_m1024_n512"

def setup_inputs():
    return {"x": np.random.randn(2048, 1024).astype(np.float32)}

def reference(x: np.ndarray) -> np.ndarray:
    return np.mean(x, axis=0, keepdims=True)
```

```python
import jax
import jax.numpy as jnp
from jax import lax
from jax.experimental import pallas as pl
from jax.experimental.pallas import tpu as pltpu

_SUBLANES = 8
_LANES = 128
_TAIL_ROWS = 128


def _tree_sum(vals):
    vals = list(vals)
    while len(vals) > 1:
        nxt = [vals[i] + vals[i + 1] for i in range(0, len(vals) - 1, 2)]
        if len(vals) % 2:
            nxt.append(vals[-1])
        vals = nxt
    return vals[0]


def _sum_row_groups(ref, ways):
    accs = [None] * ways
    for g in range(ref.shape[0] // _SUBLANES):
        v = ref[pl.ds(g * _SUBLANES, _SUBLANES), :]
        k = g % ways
        accs[k] = v if accs[k] is None else accs[k] + v
    return _tree_sum(a for a in accs if a is not None)


def pallas_dist_mean_ax0_xy_m1024_n512_kernel(
    x: jax.Array,
):
    m, n = x.shape
    tail_rows = _TAIL_ROWS
    head_rows = m - tail_rows
    cols_b = _LANES
    cols_a = n - cols_b
    x_size = lax.axis_size("x")
    assert x_size == 2, "the pairwise exchange needs an 'x' axis of size 2"
    assert head_rows > 0 and head_rows % _SUBLANES == 0
    assert cols_a > 0 and cols_a % _LANES == 0
    inv_rows = 1.0 / (x_size * m)

    def kernel_body(
        x_hbm,
        out_ref,
        head,
        tail_a,
        tail_b,
        send_a,
        send_b,
        recv_a,
        recv_b,
        load_sems,
        send_sems,
        recv_sems,
    ):
        load_head = pltpu.make_async_copy(
            x_hbm.at[pl.ds(0, head_rows)], head, load_sems.at[0]
        )
        load_a = pltpu.make_async_copy(
            x_hbm.at[pl.ds(head_rows, tail_rows), pl.ds(0, cols_a)],
            tail_a,
            load_sems.at[1],
        )
        load_b = pltpu.make_async_copy(
            x_hbm.at[pl.ds(head_rows, tail_rows), pl.ds(cols_a, cols_b)],
            tail_b,
            load_sems.at[2],
        )
        load_head.start()
        load_a.start()
        load_b.start()

        peer = (1 - lax.axis_index("x"), lax.axis_index("y"))
        barrier = pltpu.get_barrier_semaphore()
        pl.semaphore_signal(
            barrier, inc=1, device_id=peer, device_id_type=pl.DeviceIdType.MESH
        )

        swap_a = pltpu.make_async_remote_copy(
            src_ref=send_a,
            dst_ref=recv_a,
            send_sem=send_sems.at[0],
            recv_sem=recv_sems.at[0],
            device_id=peer,
            device_id_type=pl.DeviceIdType.MESH,
        )
        swap_b = pltpu.make_async_remote_copy(
            src_ref=send_b,
            dst_ref=recv_b,
            send_sem=send_sems.at[1],
            recv_sem=recv_sems.at[1],
            device_id=peer,
            device_id_type=pl.DeviceIdType.MESH,
        )

        load_head.wait()
        head_sum = _sum_row_groups(head, ways=3)

        pl.semaphore_wait(barrier, 1)

        load_a.wait()
        part_a = (
            jnp.sum(
                head_sum[:, :cols_a] + _sum_row_groups(tail_a, ways=2),
                axis=0,
                keepdims=True,
            )
            * inv_rows
        )
        send_a[...] = part_a
        swap_a.start()

        load_b.wait()
        part_b = (
            jnp.sum(
                head_sum[:, cols_a:] + _sum_row_groups(tail_b, ways=4),
                axis=0,
                keepdims=True,
            )
            * inv_rows
        )
        send_b[...] = part_b
        swap_b.start()

        swap_a.wait_send()
        swap_a.wait_recv()
        out_ref[:, pl.ds(0, cols_a)] = part_a + recv_a[...]

        swap_b.wait_send()
        swap_b.wait_recv()
        out_ref[:, pl.ds(cols_a, cols_b)] = part_b + recv_b[...]

    return pl.pallas_call(
        kernel_body,
        out_shape=jax.ShapeDtypeStruct((1, n), x.dtype),
        in_specs=[pl.BlockSpec(memory_space=pl.ANY)],
        out_specs=pl.BlockSpec(memory_space=pltpu.VMEM),
        scratch_shapes=[
            pltpu.VMEM((head_rows, n), x.dtype),
            pltpu.VMEM((tail_rows, cols_a), x.dtype),
            pltpu.VMEM((tail_rows, cols_b), x.dtype),
            pltpu.VMEM((1, cols_a), x.dtype),
            pltpu.VMEM((1, cols_b), x.dtype),
            pltpu.VMEM((1, cols_a), x.dtype),
            pltpu.VMEM((1, cols_b), x.dtype),
            pltpu.SemaphoreType.DMA((3,)),
            pltpu.SemaphoreType.DMA((2,)),
            pltpu.SemaphoreType.DMA((2,)),
        ],
        compiler_params=pltpu.CompilerParams(
            collective_id=0,
            disable_semaphore_checks=True,
        ),
        name="dist_mean_ax0_xy",
    )(x)
```

```python
import jax
import jax.numpy as jnp
from jax import lax
from jax.experimental import pallas as pl
from jax.experimental.pallas import tpu as pltpu

_SUBLANES = 8
_LANES = 128
_TAIL_ROWS = 128
_SHARED_ROWS = 32


def _tree_sum(vals):
    vals = list(vals)
    while len(vals) > 1:
        nxt = [vals[i] + vals[i + 1] for i in range(0, len(vals) - 1, 2)]
        if len(vals) % 2:
            nxt.append(vals[-1])
        vals = nxt
    return vals[0]


def _sum_row_groups(ref, ways):
    accs = [None] * ways
    for g in range(ref.shape[0] // _SUBLANES):
        v = ref[pl.ds(g * _SUBLANES, _SUBLANES), :]
        k = g % ways
        accs[k] = v if accs[k] is None else accs[k] + v
    return _tree_sum(a for a in accs if a is not None)


def pallas_dist_mean_ax0_xy_m1024_n512_kernel(
    x: jax.Array,
):
    m, n = x.shape
    tail_rows = _TAIL_ROWS
    shared_rows = _SHARED_ROWS
    head_rows = m - tail_rows - shared_rows
    cols_b = _LANES
    cols_a = n - cols_b
    x_size = lax.axis_size("x")
    assert x_size == 2, "the pairwise exchange needs an 'x' axis of size 2"
    assert head_rows > 0 and head_rows % _SUBLANES == 0
    assert cols_a > 0 and cols_a % _LANES == 0
    inv_rows = 1.0 / (x_size * m)

    def kernel_body(
        x_hbm,
        out_ref,
        head,
        tail_a,
        tail_b,
        my_shared,
        peer_shared,
        send_a,
        send_b,
        recv_a,
        recv_b,
        load_sems,
        send_sems,
        recv_sems,
    ):
        tail = pl.ds(head_rows, tail_rows)
        shared_hbm = x_hbm.at[pl.ds(head_rows + tail_rows, shared_rows)]
        load_head = pltpu.make_async_copy(
            x_hbm.at[pl.ds(0, head_rows)], head, load_sems.at[0]
        )
        load_a = pltpu.make_async_copy(
            x_hbm.at[tail, pl.ds(0, cols_a)], tail_a, load_sems.at[1]
        )
        load_b = pltpu.make_async_copy(
            x_hbm.at[tail, pl.ds(cols_a, cols_b)], tail_b, load_sems.at[2]
        )
        load_shared = pltpu.make_async_copy(shared_hbm, my_shared, load_sems.at[3])
        load_head.start()
        load_a.start()
        load_b.start()
        load_shared.start()

        peer = (1 - lax.axis_index("x"), lax.axis_index("y"))

        def to_peer(src, dst, i):
            return pltpu.make_async_remote_copy(
                src_ref=src,
                dst_ref=dst,
                send_sem=send_sems.at[i],
                recv_sem=recv_sems.at[i],
                device_id=peer,
                device_id_type=pl.DeviceIdType.MESH,
            )

        swap_shared = to_peer(shared_hbm, peer_shared, 0)
        swap_a = to_peer(send_a, recv_a, 1)
        swap_b = to_peer(send_b, recv_b, 2)

        barrier = pltpu.get_barrier_semaphore()
        pl.semaphore_signal(
            barrier, inc=1, device_id=peer, device_id_type=pl.DeviceIdType.MESH
        )
        pl.semaphore_wait(barrier, 1)
        swap_shared.start()

        load_head.wait()
        head_sum = _sum_row_groups(head, ways=3)

        load_a.wait()
        part_a = (
            jnp.sum(
                head_sum[:, :cols_a] + _sum_row_groups(tail_a, ways=2),
                axis=0,
                keepdims=True,
            )
            * inv_rows
        )
        send_a[...] = part_a
        swap_a.start()

        load_b.wait()
        part_b = (
            jnp.sum(
                head_sum[:, cols_a:] + _sum_row_groups(tail_b, ways=4),
                axis=0,
                keepdims=True,
            )
            * inv_rows
        )
        send_b[...] = part_b
        swap_b.start()

        load_shared.wait()
        swap_shared.wait_send()
        swap_shared.wait_recv()
        shared_sum = (
            jnp.sum(
                _sum_row_groups(my_shared, ways=2)
                + _sum_row_groups(peer_shared, ways=2),
                axis=0,
                keepdims=True,
            )
            * inv_rows
        )
        part_a = part_a + shared_sum[:, :cols_a]
        part_b = part_b + shared_sum[:, cols_a:]

        swap_a.wait_send()
        swap_a.wait_recv()
        out_ref[:, pl.ds(0, cols_a)] = part_a + recv_a[...]

        swap_b.wait_send()
        swap_b.wait_recv()
        out_ref[:, pl.ds(cols_a, cols_b)] = part_b + recv_b[...]

    return pl.pallas_call(
        kernel_body,
        out_shape=jax.ShapeDtypeStruct((1, n), x.dtype),
        in_specs=[pl.BlockSpec(memory_space=pl.ANY)],
        out_specs=pl.BlockSpec(memory_space=pltpu.VMEM),
        scratch_shapes=[
            pltpu.VMEM((head_rows, n), x.dtype),
            pltpu.VMEM((tail_rows, cols_a), x.dtype),
            pltpu.VMEM((tail_rows, cols_b), x.dtype),
            pltpu.VMEM((shared_rows, n), x.dtype),
            pltpu.VMEM((shared_rows, n), x.dtype),
            pltpu.VMEM((1, cols_a), x.dtype),
            pltpu.VMEM((1, cols_b), x.dtype),
            pltpu.VMEM((1, cols_a), x.dtype),
            pltpu.VMEM((1, cols_b), x.dtype),
            pltpu.SemaphoreType.DMA((4,)),
            pltpu.SemaphoreType.DMA((3,)),
            pltpu.SemaphoreType.DMA((3,)),
        ],
        compiler_params=pltpu.CompilerParams(
            collective_id=0,
            disable_semaphore_checks=True,
        ),
        name="dist_mean_ax0_xy",
    )(x)
```
